```python
import numpy as np

kernel_name = "dist_mean_ax0_shard0_i_m1024_n512"

def setup_inputs():
    return {"x": np.random.randn(4096, 512).astype(np.float32)}

def reference(x: np.ndarray) -> np.ndarray:
    return np.mean(x, axis=0, keepdims=True)
```

```python
import jax
import jax.numpy as jnp
from jax import lax
from jax.experimental import pallas as pl
from jax.experimental.pallas import tpu as pltpu

N_DEV = 4
N_CHUNKS = 8


def pallas_dist_mean_ax0_shard0_i_m1024_n512_kernel(
    x: jax.Array,
):
    m_per, n = x.shape
    m_total = m_per * N_DEV
    rows = m_per // N_CHUNKS

    def body(x_hbm, out_ref, xbuf, comm, load_sems, send_sems, recv_sems):
        me = lax.axis_index("i")

        loads = []
        for c in range(N_CHUNKS):
            cp = pltpu.make_async_copy(
                x_hbm.at[pl.ds(c * rows, rows), :],
                xbuf.at[pl.ds(c * rows, rows), :],
                load_sems.at[c],
            )
            cp.start()
            loads.append(cp)

        barrier = pltpu.get_barrier_semaphore()
        for d in range(1, N_DEV):
            pl.semaphore_signal(
                barrier,
                inc=1,
                device_id=((me + d) % N_DEV,),
                device_id_type=pl.DeviceIdType.MESH,
            )

        acc = jnp.zeros((8, n), jnp.float32)
        for c in range(N_CHUNKS):
            loads[c].wait()
            blk = xbuf[pl.ds(c * rows, rows), :]
            acc = acc + jnp.sum(blk.reshape(rows // 8, 8, n), axis=0)
        part = jnp.sum(acc, axis=0, keepdims=True)
        comm[0] = part

        pl.semaphore_wait(barrier, N_DEV - 1)

        rdmas = []
        for d in range(1, N_DEV):
            cp = pltpu.make_async_remote_copy(
                src_ref=comm.at[0],
                dst_ref=comm.at[d],
                send_sem=send_sems.at[d - 1],
                recv_sem=recv_sems.at[d - 1],
                device_id=((me + d) % N_DEV,),
                device_id_type=pl.DeviceIdType.MESH,
            )
            cp.start()
            rdmas.append(cp)

        total = part
        for d in range(1, N_DEV):
            rdmas[d - 1].wait_recv()
            total = total + comm[d]
        out_ref[...] = total * (1.0 / m_total)

        for cp in rdmas:
            cp.wait_send()

    return pl.pallas_call(
        body,
        out_shape=jax.ShapeDtypeStruct((1, n), jnp.float32),
        in_specs=[pl.BlockSpec(memory_space=pl.ANY)],
        out_specs=pl.BlockSpec(memory_space=pltpu.VMEM),
        scratch_shapes=[
            pltpu.VMEM((m_per, n), jnp.float32),
            pltpu.VMEM((N_DEV, 1, n), jnp.float32),
            pltpu.SemaphoreType.DMA((N_CHUNKS,)),
            pltpu.SemaphoreType.DMA((N_DEV - 1,)),
            pltpu.SemaphoreType.DMA((N_DEV - 1,)),
        ],
        compiler_params=pltpu.CompilerParams(collective_id=0),
    )(x)
```

```python
import jax
import jax.numpy as jnp
from jax import lax
from jax.experimental import pallas as pl
from jax.experimental.pallas import tpu as pltpu

N_DEV = 4

RAW_ROWS = 32
TAIL_ROWS = 64
LAST_MAIN_ROWS = 64
COL_GROUPS = (384, 128)


def _compiler_params():
    try:
        return pltpu.CompilerParams(collective_id=0, disable_semaphore_checks=True)
    except TypeError:
        return pltpu.CompilerParams(collective_id=0)


def _fold8(blk):
    parts = [blk[i : i + 8, :] for i in range(0, blk.shape[0], 8)]
    while len(parts) > 1:
        nxt = [parts[i] + parts[i + 1] for i in range(0, len(parts) - 1, 2)]
        if len(parts) % 2:
            nxt.append(parts[-1])
        parts = nxt
    return parts[0]


def pallas_dist_mean_ax0_shard0_i_m1024_n512_kernel(
    x: jax.Array,
):
    m, n = x.shape
    inv_total = 1.0 / (m * N_DEV)
    q0 = m - RAW_ROWS
    r0 = q0 - TAIL_ROWS
    main = ((0, r0 - LAST_MAIN_ROWS), (r0 - LAST_MAIN_ROWS, LAST_MAIN_ROWS))
    groups = []
    c0 = 0
    for cn in COL_GROUPS:
        groups.append((c0, cn))
        c0 += cn
    assert c0 == n
    ng = len(groups)

    MINE_P, NBR_A, DIAG_P, NBR_B, MINE_ALL = 0, 1, 2, 3, 4

    def body(x_hbm, out_ref, xbuf, rawbuf, comm, load_sems, send_sems, recv_sems):
        me = lax.axis_index("i")

        def peer(d):
            return dict(
                device_id=((me + d) % N_DEV,), device_id_type=pl.DeviceIdType.MESH
            )

        loads = []
        for k, (o, r) in enumerate(main):
            cp = pltpu.make_async_copy(
                x_hbm.at[pl.ds(o, r), :], xbuf.at[pl.ds(o, r), :], load_sems.at[k]
            )
            cp.start()
            loads.append(cp)
        tails = []
        for g, (co, cn) in enumerate(groups):
            cp = pltpu.make_async_copy(
                x_hbm.at[pl.ds(r0, TAIL_ROWS), pl.ds(co, cn)],
                xbuf.at[pl.ds(r0, TAIL_ROWS), pl.ds(co, cn)],
                load_sems.at[len(main) + g],
            )
            cp.start()
            tails.append(cp)

        barrier = pltpu.get_barrier_semaphore()
        for d in (2, 1, 3):
            pl.semaphore_signal(barrier, inc=1, **peer(d))
        pl.semaphore_wait(barrier, N_DEV - 1)

        raw = pltpu.make_async_remote_copy(
            src_ref=x_hbm.at[pl.ds(q0, RAW_ROWS), :],
            dst_ref=rawbuf,
            send_sem=send_sems.at[ng + 2],
            recv_sem=recv_sems.at[ng + 2],
            **peer(2),
        )
        raw.start()

        acc = None
        for k, (o, r) in enumerate(main):
            loads[k].wait()
            s = jnp.sum(xbuf[pl.ds(o, r), :].reshape(r // 8, 8, n), axis=0)
            acc = s if acc is None else acc + s

        diag = []
        for g, (co, cn) in enumerate(groups):
            tails[g].wait()
            a = acc[:, co : co + cn] + _fold8(xbuf[pl.ds(r0, TAIL_ROWS), pl.ds(co, cn)])
            comm[MINE_P, :, pl.ds(co, cn)] = jnp.sum(a, axis=0, keepdims=True)
            cp = pltpu.make_async_remote_copy(
                src_ref=comm.at[MINE_P, :, pl.ds(co, cn)],
                dst_ref=comm.at[DIAG_P, :, pl.ds(co, cn)],
                send_sem=send_sems.at[g],
                recv_sem=recv_sems.at[g],
                **peer(2),
            )
            cp.start()
            diag.append(cp)

        qload = pltpu.make_async_copy(
            x_hbm.at[pl.ds(q0, RAW_ROWS), :],
            xbuf.at[pl.ds(q0, RAW_ROWS), :],
            load_sems.at[len(main) + ng],
        )
        qload.start()
        qload.wait()
        mine = comm[MINE_P] + jnp.sum(
            _fold8(xbuf[pl.ds(q0, RAW_ROWS), :]), axis=0, keepdims=True
        )
        comm[MINE_ALL] = mine
        nbr = []
        for k, (d, slot) in enumerate(((1, NBR_A), (3, NBR_B))):
            cp = pltpu.make_async_remote_copy(
                src_ref=comm.at[MINE_ALL],
                dst_ref=comm.at[slot],
                send_sem=send_sems.at[ng + k],
                recv_sem=recv_sems.at[ng + k],
                **peer(d),
            )
            cp.start()
            nbr.append(cp)

        for cp in nbr:
            cp.wait_recv()
        base = mine + comm[NBR_A] + comm[NBR_B]
        raw.wait_recv()
        base = base + jnp.sum(_fold8(rawbuf[...]), axis=0, keepdims=True)
        for cp in diag + nbr + [raw]:
            cp.wait_send()

        for g, (co, cn) in enumerate(groups):
            diag[g].wait_recv()
            out_ref[:, pl.ds(co, cn)] = (
                base[:, co : co + cn] + comm[DIAG_P, :, pl.ds(co, cn)]
            ) * inv_total

    return pl.pallas_call(
        body,
        out_shape=jax.ShapeDtypeStruct((1, n), jnp.float32),
        in_specs=[pl.BlockSpec(memory_space=pl.ANY)],
        out_specs=pl.BlockSpec(memory_space=pltpu.VMEM),
        scratch_shapes=[
            pltpu.VMEM((m, n), jnp.float32),
            pltpu.VMEM((RAW_ROWS, n), jnp.float32),
            pltpu.VMEM((5, 1, n), jnp.float32),
            pltpu.SemaphoreType.DMA((len(main) + ng + 1,)),
            pltpu.SemaphoreType.DMA((ng + 3,)),
            pltpu.SemaphoreType.DMA((ng + 3,)),
        ],
        compiler_params=_compiler_params(),
    )(x)
```

```python
import jax
import jax.numpy as jnp
from jax import lax
from jax.experimental import pallas as pl
from jax.experimental.pallas import tpu as pltpu

N_DEV = 4

RAW_ROWS = 16
LAST_MAIN_ROWS = 64
TAIL_ROWS = 64
COL_GROUP = 128


def _compiler_params():
    try:
        return pltpu.CompilerParams(collective_id=0, disable_semaphore_checks=True)
    except TypeError:
        return pltpu.CompilerParams(collective_id=0)


def _fold8(blk):
    parts = [blk[i : i + 8, :] for i in range(0, blk.shape[0], 8)]
    while len(parts) > 1:
        nxt = [parts[i] + parts[i + 1] for i in range(0, len(parts) - 1, 2)]
        if len(parts) % 2:
            nxt.append(parts[-1])
        parts = nxt
    return parts[0]


def pallas_dist_mean_ax0_shard0_i_m1024_n512_kernel(
    x: jax.Array,
):
    m, n = x.shape
    inv_total = 1.0 / (m * N_DEV)
    m0 = 2 * RAW_ROWS
    r0 = m - TAIL_ROWS
    main = ((m0, r0 - LAST_MAIN_ROWS - m0), (r0 - LAST_MAIN_ROWS, LAST_MAIN_ROWS))
    nm = len(main)
    ng = n // COL_GROUP
    assert ng * COL_GROUP == n and all(r > 0 and r % 16 == 0 for _, r in main)

    def body(x_hbm, out_ref, xbuf, tailbuf, rawbuf, comm, load_sems, send_sems, recv_sems):
        me = lax.axis_index("i")

        def peer(d):
            return dict(
                device_id=((me + d) % N_DEV,), device_id_type=pl.DeviceIdType.MESH
            )

        def cols(g):
            return pl.ds(g * COL_GROUP, COL_GROUP)

        loads = []
        for k, (o, r) in enumerate(main):
            cp = pltpu.make_async_copy(
                x_hbm.at[pl.ds(o, r), :],
                xbuf.at[pl.ds(o - m0, r), :],
                load_sems.at[k],
            )
            cp.start()
            loads.append(cp)
        tails = []
        for g in range(ng):
            cp = pltpu.make_async_copy(
                x_hbm.at[pl.ds(r0, TAIL_ROWS), cols(g)],
                tailbuf.at[g],
                load_sems.at[nm + g],
            )
            cp.start()
            tails.append(cp)

        barrier = pltpu.get_barrier_semaphore()
        for d in (2, 1, 3):
            pl.semaphore_signal(barrier, inc=1, **peer(d))
        pl.semaphore_wait(barrier, N_DEV - 1)

        raws = []
        for k, d in enumerate((1, 3)):
            cp = pltpu.make_async_remote_copy(
                src_ref=x_hbm.at[pl.ds(k * RAW_ROWS, RAW_ROWS), :],
                dst_ref=rawbuf.at[k],
                send_sem=send_sems.at[ng + 2 + k],
                recv_sem=recv_sems.at[ng + 2 + k],
                **peer(d),
            )
            cp.start()
            raws.append(cp)

        acc = None
        for k, (o, r) in enumerate(main):
            loads[k].wait()
            s = jnp.sum(xbuf[pl.ds(o - m0, r), :].reshape(r // 16, 16, n), axis=0)
            s = s[:8] + s[8:]
            acc = s if acc is None else acc + s
            if k == 0:
                for cp in raws:
                    cp.wait_recv()
                acc = acc + (_fold8(rawbuf[0]) + _fold8(rawbuf[1]))

        diag = []
        for g in range(ng):
            tails[g].wait()
            a = acc[:, g * COL_GROUP : (g + 1) * COL_GROUP] + _fold8(tailbuf[g])
            comm[0, :, cols(g)] = jnp.sum(a, axis=0, keepdims=True)
            cp = pltpu.make_async_remote_copy(
                src_ref=comm.at[0, :, cols(g)],
                dst_ref=comm.at[2, :, cols(g)],
                send_sem=send_sems.at[g],
                recv_sem=recv_sems.at[g],
                **peer(2),
            )
            cp.start()
            diag.append(cp)

        nbr = []
        for k, d in enumerate((1, 3)):
            cp = pltpu.make_async_remote_copy(
                src_ref=comm.at[0],
                dst_ref=comm.at[d],
                send_sem=send_sems.at[ng + k],
                recv_sem=recv_sems.at[ng + k],
                **peer(d),
            )
            cp.start()
            nbr.append(cp)

        for cp in nbr:
            cp.wait_recv()
        base = comm[0] + comm[1] + comm[3]
        for cp in raws + diag + nbr:
            cp.wait_send()

        for g in range(ng):
            diag[g].wait_recv()
            out_ref[:, cols(g)] = (
                base[:, g * COL_GROUP : (g + 1) * COL_GROUP] + comm[2, :, cols(g)]
            ) * inv_total

    return pl.pallas_call(
        body,
        out_shape=jax.ShapeDtypeStruct((1, n), jnp.float32),
        in_specs=[pl.BlockSpec(memory_space=pl.ANY)],
        out_specs=pl.BlockSpec(memory_space=pltpu.VMEM),
        scratch_shapes=[
            pltpu.VMEM((r0 - m0, n), jnp.float32),
            pltpu.VMEM((ng, TAIL_ROWS, COL_GROUP), jnp.float32),
            pltpu.VMEM((2, RAW_ROWS, n), jnp.float32),
            pltpu.VMEM((N_DEV, 1, n), jnp.float32),
            pltpu.SemaphoreType.DMA((nm + ng,)),
            pltpu.SemaphoreType.DMA((ng + 4,)),
            pltpu.SemaphoreType.DMA((ng + 4,)),
        ],
        compiler_params=_compiler_params(),
    )(x)
```

```python
import jax
import jax.numpy as jnp
from jax import lax
from jax.experimental import pallas as pl
from jax.experimental.pallas import tpu as pltpu

N_DEV = 4

RAW_ROWS = 16
LAST_MAIN_ROWS = 64
TAIL_ROWS = 64
COL_GROUP = 128


def _compiler_params():
    try:
        return pltpu.CompilerParams(collective_id=0, disable_semaphore_checks=True)
    except TypeError:
        return pltpu.CompilerParams(collective_id=0)


def _fold8(blk):
    parts = [blk[i : i + 8, :] for i in range(0, blk.shape[0], 8)]
    while len(parts) > 1:
        nxt = [parts[i] + parts[i + 1] for i in range(0, len(parts) - 1, 2)]
        if len(parts) % 2:
            nxt.append(parts[-1])
        parts = nxt
    return parts[0]


def pallas_dist_mean_ax0_shard0_i_m1024_n512_kernel(
    x: jax.Array,
):
    m, n = x.shape
    inv_total = 1.0 / (m * N_DEV)
    m0 = 2 * RAW_ROWS
    r0 = m - TAIL_ROWS
    main = ((m0, r0 - LAST_MAIN_ROWS - m0), (r0 - LAST_MAIN_ROWS, LAST_MAIN_ROWS))
    nm = len(main)
    ng = n // COL_GROUP
    assert ng * COL_GROUP == n and all(r > 0 and r % 16 == 0 for _, r in main)

    def body(x_hbm, out_ref, xbuf, tailbuf, rawbuf, comm, load_sems, send_sems, recv_sems):
        me = lax.axis_index("i")

        def peer(d):
            return dict(
                device_id=((me + d) % N_DEV,), device_id_type=pl.DeviceIdType.MESH
            )

        def cols(g):
            return pl.ds(g * COL_GROUP, COL_GROUP)

        loads = []
        for k, (o, r) in enumerate(main):
            cp = pltpu.make_async_copy(
                x_hbm.at[pl.ds(o, r), :],
                xbuf.at[pl.ds(o - m0, r), :],
                load_sems.at[k],
            )
            cp.start()
            loads.append(cp)
        tails = []
        for g in range(ng):
            cp = pltpu.make_async_copy(
                x_hbm.at[pl.ds(r0, TAIL_ROWS), cols(g)],
                tailbuf.at[g],
                load_sems.at[nm + g],
            )
            cp.start()
            tails.append(cp)

        barrier = pltpu.get_barrier_semaphore()
        for d in (2, 1, 3):
            pl.semaphore_signal(barrier, inc=1, **peer(d))
        pl.semaphore_wait(barrier, N_DEV - 1)

        raws = []
        for k, d in enumerate((1, 3)):
            cp = pltpu.make_async_remote_copy(
                src_ref=x_hbm.at[pl.ds(k * RAW_ROWS, RAW_ROWS), :],
                dst_ref=rawbuf.at[k],
                send_sem=send_sems.at[ng + 2 + k],
                recv_sem=recv_sems.at[ng + 2 + k],
                **peer(d),
            )
            cp.start()
            raws.append(cp)

        acc = None
        for k, (o, r) in enumerate(main):
            loads[k].wait()
            s = jnp.sum(xbuf[pl.ds(o - m0, r), :].reshape(r // 16, 16, n), axis=0)
            s = s[:8] + s[8:]
            acc = s if acc is None else acc + s
            if k == 0:
                for cp in raws:
                    cp.wait_recv()
                acc = acc + (_fold8(rawbuf[0]) + _fold8(rawbuf[1]))

        diag = []
        for g in range(ng):
            tails[g].wait()
            a = acc[:, g * COL_GROUP : (g + 1) * COL_GROUP] + _fold8(tailbuf[g])
            comm[0, g] = jnp.sum(a, axis=0, keepdims=True)
            cp = pltpu.make_async_remote_copy(
                src_ref=comm.at[0, g],
                dst_ref=comm.at[2, g],
                send_sem=send_sems.at[g],
                recv_sem=recv_sems.at[g],
                **peer(2),
            )
            cp.start()
            diag.append(cp)

        nbr = []
        for k, d in enumerate((1, 3)):
            cp = pltpu.make_async_remote_copy(
                src_ref=comm.at[0],
                dst_ref=comm.at[d],
                send_sem=send_sems.at[ng + k],
                recv_sem=recv_sems.at[ng + k],
                **peer(d),
            )
            cp.start()
            nbr.append(cp)

        for cp in nbr:
            cp.wait_recv()
        base = [comm[0, g] + comm[1, g] + comm[3, g] for g in range(ng)]
        for cp in raws + diag + nbr:
            cp.wait_send()

        for g in range(ng):
            diag[g].wait_recv()
            out_ref[:, cols(g)] = (base[g] + comm[2, g]) * inv_total

    return pl.pallas_call(
        body,
        out_shape=jax.ShapeDtypeStruct((1, n), jnp.float32),
        in_specs=[pl.BlockSpec(memory_space=pl.ANY)],
        out_specs=pl.BlockSpec(memory_space=pltpu.VMEM),
        scratch_shapes=[
            pltpu.VMEM((r0 - m0, n), jnp.float32),
            pltpu.VMEM((ng, TAIL_ROWS, COL_GROUP), jnp.float32),
            pltpu.VMEM((2, RAW_ROWS, n), jnp.float32),
            pltpu.VMEM((N_DEV, ng, 1, COL_GROUP), jnp.float32),
            pltpu.SemaphoreType.DMA((nm + ng,)),
            pltpu.SemaphoreType.DMA((ng + 4,)),
            pltpu.SemaphoreType.DMA((ng + 4,)),
        ],
        compiler_params=_compiler_params(),
    )(x)
```

```python
import jax
import jax.numpy as jnp
from jax import lax
from jax.experimental import pallas as pl
from jax.experimental.pallas import tpu as pltpu

N_DEV = 4

RAW_ROWS = 16
LAST_MAIN_ROWS = 64
TAIL_ROWS = 64
COL_GROUP = 128


def _compiler_params():
    try:
        return pltpu.CompilerParams(collective_id=0, disable_semaphore_checks=True)
    except TypeError:
        return pltpu.CompilerParams(collective_id=0)


def _fold8(blk):
    parts = [blk[i : i + 8, :] for i in range(0, blk.shape[0], 8)]
    while len(parts) > 1:
        nxt = [parts[i] + parts[i + 1] for i in range(0, len(parts) - 1, 2)]
        if len(parts) % 2:
            nxt.append(parts[-1])
        parts = nxt
    return parts[0]


def pallas_dist_mean_ax0_shard0_i_m1024_n512_kernel(
    x: jax.Array,
):
    m, n = x.shape
    inv_total = 1.0 / (m * N_DEV)
    m0 = 2 * RAW_ROWS
    r0 = m - TAIL_ROWS
    main = ((m0, r0 - LAST_MAIN_ROWS - m0), (r0 - LAST_MAIN_ROWS, LAST_MAIN_ROWS))
    nm = len(main)
    ng = n // COL_GROUP
    assert ng * COL_GROUP == n and all(r > 0 and r % 16 == 0 for _, r in main)

    def body(x_hbm, out_ref, xbuf, tailbuf, rawbuf, comm, load_sems, send_sems, recv_sems):
        me = lax.axis_index("i")

        def peer(d):
            return dict(
                device_id=((me + d) % N_DEV,), device_id_type=pl.DeviceIdType.MESH
            )

        def cols(g):
            return pl.ds(g * COL_GROUP, COL_GROUP)

        loads = []
        for k, (o, r) in enumerate(main):
            cp = pltpu.make_async_copy(
                x_hbm.at[pl.ds(o, r), :],
                xbuf.at[pl.ds(o - m0, r), :],
                load_sems.at[k],
            )
            cp.start()
            loads.append(cp)
        tails = []
        for g in range(ng):
            cp = pltpu.make_async_copy(
                x_hbm.at[pl.ds(r0, TAIL_ROWS), cols(g)],
                tailbuf.at[g],
                load_sems.at[nm + g],
            )
            cp.start()
            tails.append(cp)

        barrier = pltpu.get_barrier_semaphore()
        for d in (2, 1, 3):
            pl.semaphore_signal(barrier, inc=1, **peer(d))
        pl.semaphore_wait(barrier, N_DEV - 1)

        raws = []
        for k, d in enumerate((1, 3)):
            cp = pltpu.make_async_remote_copy(
                src_ref=x_hbm.at[pl.ds(k * RAW_ROWS, RAW_ROWS), :],
                dst_ref=rawbuf.at[k],
                send_sem=send_sems.at[ng + 2 + k],
                recv_sem=recv_sems.at[ng + 2 + k],
                **peer(d),
            )
            cp.start()
            raws.append(cp)

        acc = None
        for k, (o, r) in enumerate(main):
            loads[k].wait()
            s = jnp.sum(xbuf[pl.ds(o - m0, r), :].reshape(r // 16, 16, n), axis=0)
            s = s[:8] + s[8:]
            acc = s if acc is None else acc + s
        for cp in raws:
            cp.wait_recv()
        acc = acc + (_fold8(rawbuf[0]) + _fold8(rawbuf[1]))

        diag = []
        for g in range(ng):
            tails[g].wait()
            a = acc[:, g * COL_GROUP : (g + 1) * COL_GROUP] + _fold8(tailbuf[g])
            comm[0, g] = jnp.sum(a, axis=0, keepdims=True)
            cp = pltpu.make_async_remote_copy(
                src_ref=comm.at[0, g],
                dst_ref=comm.at[2, g],
                send_sem=send_sems.at[g],
                recv_sem=recv_sems.at[g],
                **peer(2),
            )
            cp.start()
            diag.append(cp)

        nbr = []
        for k, d in enumerate((1, 3)):
            cp = pltpu.make_async_remote_copy(
                src_ref=comm.at[0],
                dst_ref=comm.at[d],
                send_sem=send_sems.at[ng + k],
                recv_sem=recv_sems.at[ng + k],
                **peer(d),
            )
            cp.start()
            nbr.append(cp)

        for cp in nbr:
            cp.wait_recv()
        base = [comm[0, g] + comm[1, g] + comm[3, g] for g in range(ng)]
        for cp in raws + diag + nbr:
            cp.wait_send()

        for g in range(ng):
            diag[g].wait_recv()
            out_ref[:, cols(g)] = (base[g] + comm[2, g]) * inv_total

    return pl.pallas_call(
        body,
        out_shape=jax.ShapeDtypeStruct((1, n), jnp.float32),
        in_specs=[pl.BlockSpec(memory_space=pl.ANY)],
        out_specs=pl.BlockSpec(memory_space=pltpu.VMEM),
        scratch_shapes=[
            pltpu.VMEM((r0 - m0, n), jnp.float32),
            pltpu.VMEM((ng, TAIL_ROWS, COL_GROUP), jnp.float32),
            pltpu.VMEM((2, RAW_ROWS, n), jnp.float32),
            pltpu.VMEM((N_DEV, ng, 1, COL_GROUP), jnp.float32),
            pltpu.SemaphoreType.DMA((nm + ng,)),
            pltpu.SemaphoreType.DMA((ng + 4,)),
            pltpu.SemaphoreType.DMA((ng + 4,)),
        ],
        compiler_params=_compiler_params(),
    )(x)
```
